```python
import numpy as np

kernel_name = "dist_max_ax1_xy_m2048_n1024"

def setup_inputs():
    return {"x": np.random.randn(4096, 2048).astype(np.float32)}

def reference(x: np.ndarray) -> np.ndarray:
    return np.max(x, axis=1, keepdims=True)
```

```python
import jax
import jax.numpy as jnp
from jax import lax
from jax.experimental import pallas as pl
from jax.experimental.pallas import tpu as pltpu

M, N = 2048, 1024
NB = M // 128
NEG = float("-inf")

RS = 48
CHUNKS = (256 - RS, 256, 256, 256, 256, 256, 256, 128, 96, 24, 8)
STARTS = tuple(RS + sum(CHUNKS[:c]) for c in range(len(CHUNKS)))
NCH = len(CHUNKS)
BOUNCE_AFTER = 3
SMEM_ROWS_AFTER = 6
DEFER = 1
assert sum(CHUNKS) == M - RS


def pallas_dist_max_ax1_xy_m2048_n1024_kernel(x: jax.Array):
    def body(x_hbm, out_ref, xbuf, sbuf, part, recv, in_sems, sm_sems, send_sems, recv_sems):
        def load(c):
            rows = pl.ds(STARTS[c], CHUNKS[c])
            return pltpu.make_async_copy(x_hbm.at[rows], xbuf.at[rows], in_sems.at[c])

        sm_in = pltpu.make_async_copy(x_hbm.at[pl.ds(0, RS)], sbuf, sm_sems.at[0])
        sm_out = pltpu.make_async_copy(sbuf, xbuf.at[pl.ds(0, RS)], sm_sems.at[1])

        load(0).start()
        sm_in.start()
        for c in range(1, NCH):
            load(c).start()

        nbr = (lax.axis_index("x"), 1 - lax.axis_index("y"))
        barrier = pltpu.get_barrier_semaphore()
        pl.semaphore_signal(barrier, inc=1, device_id=nbr, device_id_type=pl.DeviceIdType.MESH)

        def exchange(i, b0, nb):
            rows = pl.ds(b0, nb)
            return pltpu.make_async_remote_copy(
                src_ref=part.at[rows], dst_ref=recv.at[rows],
                send_sem=send_sems.at[i], recv_sem=recv_sems.at[i],
                device_id=nbr, device_id_type=pl.DeviceIdType.MESH)

        lane = lax.broadcasted_iota(jnp.int32, (8, 128), 1)
        sub = lax.broadcasted_iota(jnp.int32, (8, 128), 0)
        diag = (lane & 7) == sub
        grp = lane >> 3

        def fold_columns(g):
            v = [xbuf[pl.ds(g * 8, 8), pl.ds(j * 128, 128)] for j in range(N // 128)]
            while len(v) > 1:
                v = [jnp.maximum(v[2 * i], v[2 * i + 1]) for i in range(len(v) // 2)]
            return v[0]

        accs, counts = {}, {}

        def fold_lanes(g, m):
            b, gi = g // 16, g % 16
            col = jnp.broadcast_to(jnp.max(m, axis=1, keepdims=True), (8, 128))
            accs[b] = col if b not in accs else jnp.where(grp == gi, col, accs[b])
            counts[b] = counts.get(b, 0) + 1
            if counts[b] == 16:
                part[pl.ds(b, 1), :] = jnp.max(
                    jnp.where(diag, accs.pop(b), NEG), axis=0, keepdims=True)

        pending = []
        for c in range(NCH):
            load(c).wait()
            pending += [(g, fold_columns(g))
                        for g in range(STARTS[c] // 8, (STARTS[c] + CHUNKS[c]) // 8)]
            if not (NCH - 1 - DEFER <= c < NCH - 1):
                for g, m in pending:
                    fold_lanes(g, m)
                pending = []
            if c == BOUNCE_AFTER:
                sm_in.wait()
                sm_out.start()
            if c == SMEM_ROWS_AFTER:
                sm_out.wait()
                for g in range(RS // 8):
                    fold_lanes(g, fold_columns(g))
            if STARTS[c] + CHUNKS[c] == M - 128:
                pl.semaphore_wait(barrier, 1)
                exchange(0, 0, NB - 1).start()
        exchange(1, NB - 1, 1).start()
        exchange(0, 0, NB - 1).wait()
        exchange(1, NB - 1, 1).wait()
        out_ref[...] = jnp.maximum(part[...], recv[...])

    out = pl.pallas_call(
        body,
        out_shape=jax.ShapeDtypeStruct((NB, 128), jnp.float32),
        in_specs=[pl.BlockSpec(memory_space=pl.ANY)],
        out_specs=pl.BlockSpec(memory_space=pltpu.VMEM),
        scratch_shapes=[
            pltpu.VMEM((M, N), jnp.float32),
            pltpu.SMEM((RS, N), jnp.float32),
            pltpu.VMEM((NB, 128), jnp.float32),
            pltpu.VMEM((NB, 128), jnp.float32),
            pltpu.SemaphoreType.DMA((NCH,)),
            pltpu.SemaphoreType.DMA((2,)),
            pltpu.SemaphoreType.DMA((2,)),
            pltpu.SemaphoreType.DMA((2,)),
        ],
        compiler_params=pltpu.CompilerParams(
            collective_id=0, disable_semaphore_checks=True, disable_bounds_checks=True),
    )(x)
    return out.reshape(M, 1)
```

```python
import jax
import jax.numpy as jnp
from jax import lax
from jax.experimental import pallas as pl
from jax.experimental.pallas import tpu as pltpu

M, N = 2048, 1024
NB = M // 128
NT = N // 128
NEG = float("-inf")
MESH = pl.DeviceIdType.MESH

def make(RY=112, RX=0, RS=0, TAIL=(96, 16, 8, 8), POP=(0, 3, 3, 3), KCH=3, EX1_AT=0, ZORD=(0, -1, 1, -2), ZLEN=9, NDUM=2, ORD2=(2, 3, 0, 1),
         BOUNCE_AFTER=6, SM_PROC_AFTER=13, X_AFTER=12, PROF=0, SM_START=-1):
    special = [RY] + ([RX] if RX else []) + ([RS] if RS else [])
    assert special == sorted(special, reverse=True)
    XB = 1; SB = 2 if RX else 1
    a0 = [sum(1 for r in special if 8 * b < r) for b in range(16)]
    NTL = len(TAIL)
    K = sum(TAIL[NTL - KCH:])
    tstart = [sum(TAIL[:r]) for r in range(NTL)]

    def kernel(x):
        def body(x_hbm, out_ref, xbuf, yraw, xraw, sbuf, part, recv, part2, srecv, px, pxo, pxn,
                 in_sems, tl_sems, sm_sems, own_sem, send_sems, recv_sems, ready):
            def sweep(b):
                idx = (pl.ds(a0[b], NB - 1 - a0[b]), pl.ds(8 * b, 8))
                return pltpu.make_async_copy(x_hbm.at[idx], xbuf.at[idx], in_sems.at[b])
            def tail(r):
                idx = (NB - 1, pl.ds(tstart[r], TAIL[r]))
                return pltpu.make_async_copy(x_hbm.at[idx], xbuf.at[idx], tl_sems.at[r])
            if RS:
                sm_in = pltpu.make_async_copy(x_hbm.at[SB, pl.ds(0, RS)], sbuf, sm_sems.at[0])
                sm_out = pltpu.make_async_copy(sbuf, xbuf.at[SB, pl.ds(0, RS)], sm_sems.at[1])
            sweep(0).start()
            if RS and SM_START < 0: sm_in.start()
            for b in range(1, 16): sweep(b).start()
            for r in range(NTL): tail(r).start()
            mx = lax.axis_index("x"); my = lax.axis_index("y")
            ynbr = (mx, 1 - my); xnbr = (1 - mx, my); diagd = (1 - mx, 1 - my)
            bar = pltpu.get_barrier_semaphore()
            pl.semaphore_signal(bar, inc=1, device_id=ynbr, device_id_type=MESH)
            if RX:
                @pl.when(mx == 0)
                def _():
                    pl.semaphore_signal(bar, inc=1, device_id=xnbr, device_id_type=MESH)
                    pl.semaphore_wait(bar, 1)
                @pl.when(mx == 1)
                def _():
                    pl.semaphore_wait(bar, 2)
                    pl.semaphore_signal(ready, inc=1, device_id=xnbr, device_id_type=MESH)
            else:
                pl.semaphore_wait(bar, 1)
            def remote(i, src, dst, dev):
                return pltpu.make_async_remote_copy(src_ref=src, dst_ref=dst,
                    send_sem=send_sems.at[i], recv_sem=recv_sems.at[i], device_id=dev, device_id_type=MESH)
            ex0 = lambda: remote(0, part.at[pl.ds(0, NB - 1)], recv.at[pl.ds(0, NB - 1)], ynbr)
            ex1 = lambda: remote(1, part.at[pl.ds(NB - 1, 1)], recv.at[pl.ds(NB - 1, 1)], ynbr)
            ex2 = lambda: remote(2, part2, srecv, ynbr)
            rawy = lambda: remote(3, x_hbm.at[0, pl.ds(0, RY)], yraw, ynbr)
            rawx = lambda: remote(4, x_hbm.at[XB, pl.ds(0, RX)], xraw, xnbr)
            pxd = lambda: remote(5, px, pxn, diagd)
            pxb = lambda: remote(6, px, pxo, xnbr)
            own = pltpu.make_async_copy(x_hbm.at[0, pl.ds(0, RY)], xbuf.at[0, pl.ds(0, RY)], own_sem)
            rawy().start()
            if RX:
                @pl.when(mx == 0)
                def _():
                    pl.semaphore_wait(ready, 1)
                rawx().start()

            lane = lax.broadcasted_iota(jnp.int32, (8, 128), 1)
            sub = lax.broadcasted_iota(jnp.int32, (8, 128), 0)
            grp = lane >> 3
            bits = [(lane & b) != 0 for b in (1, 2, 4)]
            negs = jnp.full((8, 128), NEG, jnp.float32)

            def tree(v):
                while len(v) > 1:
                    v = [jnp.maximum(v[2 * i], v[2 * i + 1]) for i in range(len(v) // 2)] + ([v[-1]] if len(v) % 2 else [])
                return v[0]
            def fold(ref, g):
                return tree([ref[pl.ds(g * 8, 8), pl.ds(j * 128, 128)] for j in range(NT)])
            def xl(m):
                return jnp.broadcast_to(jnp.max(m, axis=1, keepdims=True), (8, 128))
            def to_row(acc):
                rs = [acc] + [pltpu.roll(acc, 8 - k, 0) for k in range(1, 8)]
                for bm in bits:
                    rs = [jnp.where(bm, rs[2 * i + 1], rs[2 * i]) for i in range(len(rs) // 2)]
                return rs[0][0:1, :]
            def to_rows(v):
                for bit in (4, 2, 1):
                    sb = (sub & bit) != 0
                    same = sb == ((lane & bit) != 0)
                    nv = []
                    for a in range(bit):
                        X, Y = v[a], v[a + bit]
                        stay = jnp.where(sb, Y, X)
                        U = jnp.where(sb, X, Y)
                        if bit == 4:
                            mv = pltpu.roll(U, 4, 0)
                        else:
                            mv = jnp.where(sb, pltpu.roll(U, bit, 0), pltpu.roll(U, 8 - bit, 0))
                        nv.append(jnp.where(same, stay, mv))
                    v = nv
                return v[0]

            accs = [negs] * 16
            for b in range(16):
                sweep(b).wait()
                gm = grp == b
                for a in range(a0[b], NB - 1):
                    accs[a] = jnp.where(gm, xl(fold(xbuf.at[a], b)), accs[a])
                if RS and b == SM_START:
                    sm_in.start()
                if RS and b == BOUNCE_AFTER:
                    sm_in.wait(); sm_out.start()
                if RX and b == X_AFTER:
                    rawx().wait_recv()
                    acc = negs
                    for g in range(RX // 8):
                        acc = jnp.where(grp == g, xl(fold(xraw, g)), acc)
                    px[...] = to_row(acc)
                    pxd().start(); pxb().start()
                if RS and b == SM_PROC_AFTER:
                    sm_out.wait()
                    for g in range(RS // 8):
                        accs[SB] = jnp.where(grp == g, xl(fold(xbuf.at[SB], g)), accs[SB])
            part[pl.ds(0, 8), :] = to_rows(accs[:8])
            part[pl.ds(8, 7), :] = to_rows(accs[8:])[0:7, :]
            ex0().start()

            xl5 = xbuf.at[NB - 1]
            folded = {}
            acc1 = negs
            cols2 = []
            zrow = None
            for r in range(NTL):
                tail(r).wait()
                folded[r] = [(g, fold(xl5, g)) for g in range(tstart[r] // 8, (tstart[r] + TAIL[r]) // 8)]
                if r == NTL - 2 and NDUM:
                    keep = [(i, xl5[pl.ds(8 * i, 8), pl.ds(0, 128)]) for i in range(NDUM)]
                allc = []
                for c in range(r + 1):
                    if POP[c] == r:
                        for gi, m in folded[c]:
                            cb = xl(m)
                            allc.append((gi, cb))
                            if c < NTL - KCH:
                                acc1 = jnp.where(grp == gi, cb, acc1)
                            else:
                                cols2.append((gi, cb))
                if r == NTL - 1 and ZORD is not None:
                    dc = [(gi, xl(m)) for gi, m in keep] if NDUM else []
                    z = negs
                    for o in ZORD:
                        gi, cb = allc[o] if o >= 0 else dc[-o - 1]
                        z = jnp.maximum(z, jnp.where(lane == sub + gi * 8, cb, NEG))
                    for q in range(ZLEN):
                        z = jnp.maximum(z, pltpu.roll(z, (4, 2, 1)[q % 3], 0))
                    zrow = z[0:1, :]
                if r == EX1_AT:
                    part[pl.ds(NB - 1, 1), :] = to_row(acc1)
                    ex1().start()
            acc2 = negs
            for o in (ORD2 if ORD2 is not None else range(len(cols2))):
                gi, cb = cols2[o]
                acc2 = jnp.where(grp == gi, cb, acc2)
            part2[...] = to_row(acc2)
            ex2().start()
            own.start()
            own.wait()
            rawy().wait_recv()
            acc = negs
            for g in range(RY // 8):
                acc = jnp.where(grp == g, xl(jnp.maximum(fold(xbuf.at[0], g), fold(yraw, g))), acc)
            row0 = to_row(acc)
            rawy().wait_send()
            ex0().wait()
            lo = jnp.maximum(part[pl.ds(0, 8), :], recv[pl.ds(0, 8), :])
            lo = jnp.maximum(lo, jnp.where(sub == 0, jnp.broadcast_to(row0, (8, 128)), NEG))
            if RX:
                rawx().wait_send()
                pxd().wait(); pxb().wait()
                row1 = jnp.maximum(pxo[...], pxn[...])
                lo = jnp.maximum(lo, jnp.where(sub == XB, jnp.broadcast_to(row1, (8, 128)), NEG))
            out_ref[pl.ds(0, 8), :] = lo
            out_ref[pl.ds(8, 7), :] = jnp.maximum(part[pl.ds(8, 7), :], recv[pl.ds(8, 7), :])
            last = jnp.maximum(part[pl.ds(NB - 1, 1), :], part2[...])
            if zrow is not None:
                last = jnp.maximum(last, zrow)
            ex1().wait_send()
            ex2().wait_send()
            l1 = lax.broadcasted_iota(jnp.int32, (1, 128), 1)
            ex1().wait_recv()
            last = jnp.maximum(last, recv[pl.ds(NB - 1, 1), :])
            ex2().wait_recv()
            a2 = last
            for i in range(128 - K, 128):
                a2 = jnp.where(l1 == i, srecv[0, i], a2)
            out_ref[pl.ds(NB - 1, 1), :] = jnp.maximum(last, a2)

        row = pltpu.VMEM((1, 128), jnp.float32)
        out = pl.pallas_call(
            body,
            out_shape=jax.ShapeDtypeStruct((NB, 128), jnp.float32),
            in_specs=[pl.BlockSpec(memory_space=pl.ANY)],
            out_specs=pl.BlockSpec(memory_space=pltpu.VMEM),
            scratch_shapes=[
                pltpu.VMEM((NB, 128, N), jnp.float32),
                pltpu.VMEM((RY, N), jnp.float32),
                pltpu.VMEM((max(RX, 8), N), jnp.float32),
                pltpu.SMEM((max(RS, 8), N), jnp.float32),
                pltpu.VMEM((NB, 128), jnp.float32),
                pltpu.VMEM((NB, 128), jnp.float32),
                row,
                pltpu.SMEM((1, 128), jnp.float32),
                row, row, row,
                pltpu.SemaphoreType.DMA((16,)),
                pltpu.SemaphoreType.DMA((NTL,)),
                pltpu.SemaphoreType.DMA((2,)),
                pltpu.SemaphoreType.DMA,
                pltpu.SemaphoreType.DMA((7,)),
                pltpu.SemaphoreType.DMA((7,)),
                pltpu.SemaphoreType.REGULAR,
            ],
            compiler_params=pltpu.CompilerParams(collective_id=0, disable_semaphore_checks=True, disable_bounds_checks=True),
        )(x.reshape(NB, 128, N))
        return out.reshape(M, 1)
    return kernel

pallas_dist_max_ax1_xy_m2048_n1024_kernel = make()
```

```python
import jax
import jax.numpy as jnp
from jax import lax
from jax.experimental import pallas as pl
from jax.experimental.pallas import tpu as pltpu

M, N = 2048, 1024
NB = M // 128
NG = 16
NT = N // 128
NEG = float("-inf")
MESH = pl.DeviceIdType.MESH

RY = 112
RX = 56
RF = 16
FIRST = tuple((8 * b < RY) + (8 * b < RX) for b in range(NG))
EARLY = 6
FWD_AFTER = 2
X_AFTER = 11
TAIL = ((0, 96), (96, 16), (112, 8), (120, 8))
K = 32


def pallas_dist_max_ax1_xy_m2048_n1024_kernel(x: jax.Array):
    def body(x_hbm, out_ref, xbuf, yraw, xraw, stage, part, recv, last_s, last_r, px_s, px_r,
             sweep_sems, tail_sems, misc_sems, send_sems, recv_sems, ready):
        def sweep(b):
            idx = (pl.ds(FIRST[b], NB - 1 - FIRST[b]), pl.ds(8 * b, 8))
            return pltpu.make_async_copy(x_hbm.at[idx], xbuf.at[idx], sweep_sems.at[b])

        def tail(r):
            idx = (NB - 1, pl.ds(*TAIL[r]))
            return pltpu.make_async_copy(x_hbm.at[idx], xbuf.at[idx], tail_sems.at[r])

        stage_in = pltpu.make_async_copy(x_hbm.at[1, pl.ds(RX - RF, RF)], stage, misc_sems.at[0])
        reread = pltpu.make_async_copy(
            x_hbm.at[0, pl.ds(0, RY)], xbuf.at[0, pl.ds(0, RY)], misc_sems.at[1])

        sweep(0).start()
        stage_in.start()
        for b in range(1, EARLY):
            sweep(b).start()

        mx, my = lax.axis_index("x"), lax.axis_index("y")
        ynbr, xnbr = (mx, 1 - my), (1 - mx, my)
        barrier = pltpu.get_barrier_semaphore()
        pl.semaphore_signal(barrier, inc=1, device_id=ynbr, device_id_type=MESH)

        @pl.when(mx == 0)
        def _():
            pl.semaphore_signal(barrier, inc=1, device_id=xnbr, device_id_type=MESH)
            pl.semaphore_wait(barrier, 1)

        @pl.when(mx == 1)
        def _():
            pl.semaphore_wait(barrier, 2)
            pl.semaphore_signal(ready, inc=1, device_id=xnbr, device_id_type=MESH)

        def remote(i, src, dst, dev):
            return pltpu.make_async_remote_copy(
                src_ref=src, dst_ref=dst, send_sem=send_sems.at[i], recv_sem=recv_sems.at[i],
                device_id=dev, device_id_type=MESH)

        raw_y = remote(0, x_hbm.at[0, pl.ds(0, RY)], yraw, ynbr)
        raw_x = remote(1, x_hbm.at[1, pl.ds(0, RX - RF)], xraw.at[pl.ds(0, RX - RF)], xnbr)
        fwd_x = remote(2, stage, xraw.at[pl.ds(RX - RF, RF)], xnbr)
        back_x = remote(3, px_s, px_r, xnbr)
        ex0 = remote(4, part.at[pl.ds(0, NB - 1)], recv.at[pl.ds(0, NB - 1)], ynbr)
        ex1 = remote(5, part.at[pl.ds(NB - 1, 1)], recv.at[pl.ds(NB - 1, 1)], ynbr)
        ex2 = remote(6, last_s, last_r, ynbr)

        raw_y.start()
        for b in range(EARLY, NG):
            sweep(b).start()
        for r in range(len(TAIL)):
            tail(r).start()

        @pl.when(mx == 0)
        def _():
            pl.semaphore_wait(ready, 1)

        raw_x.start()

        lane = lax.broadcasted_iota(jnp.int32, (8, 128), 1)
        sub = lax.broadcasted_iota(jnp.int32, (8, 128), 0)
        grp = lane >> 3
        negs = jnp.full((8, 128), NEG, jnp.float32)

        def fold(ref, g):
            v = [ref[pl.ds(g * 8, 8), pl.ds(j * 128, 128)] for j in range(NT)]
            while len(v) > 1:
                v = [jnp.maximum(v[2 * i], v[2 * i + 1]) for i in range(len(v) // 2)]
            return v[0]

        def row_max(m):
            return jnp.broadcast_to(jnp.max(m, axis=1, keepdims=True), (8, 128))

        def to_row(acc):
            rs = [acc] + [pltpu.roll(acc, 8 - k, 0) for k in range(1, 8)]
            for bit in (1, 2, 4):
                odd = (lane & bit) != 0
                rs = [jnp.where(odd, rs[2 * i + 1], rs[2 * i]) for i in range(len(rs) // 2)]
            return rs[0][0:1, :]

        def to_rows(v):
            for bit in (4, 2, 1):
                hi = (sub & bit) != 0
                same = hi == ((lane & bit) != 0)
                nv = []
                for a in range(bit):
                    stay = jnp.where(hi, v[a + bit], v[a])
                    move = jnp.where(hi, v[a], v[a + bit])
                    if bit == 4:
                        move = pltpu.roll(move, 4, 0)
                    else:
                        move = jnp.where(hi, pltpu.roll(move, bit, 0), pltpu.roll(move, 8 - bit, 0))
                    nv.append(jnp.where(same, stay, move))
                v = nv
            return v[0]

        def as_row(row, a):
            return jnp.where(sub == a, jnp.broadcast_to(row, (8, 128)), NEG)

        accs = [negs] * NB
        for b in range(NG):
            sweep(b).wait()
            if b == NG - 1:
                back_x.wait_recv()
            for a in range(FIRST[b], NB - 1):
                accs[a] = jnp.where(grp == b, row_max(fold(xbuf.at[a], b)), accs[a])
            if b == FWD_AFTER:
                stage_in.wait()
                fwd_x.start()
            if b == X_AFTER:
                raw_x.wait_recv()
                fwd_x.wait_recv()
                acc = negs
                for g in range(RX // 8):
                    acc = jnp.where(grp == g, row_max(fold(xraw, g)), acc)
                px_s[...] = to_row(acc)
                back_x.start()
        part[pl.ds(0, 8), :] = jnp.maximum(to_rows(accs[:8]), as_row(px_r[...], 1))
        part[pl.ds(8, 7), :] = to_rows(accs[8:])[0:7, :]
        ex0.start()

        blk = xbuf.at[NB - 1]
        tail(0).wait()
        acc = negs
        for g in range(12):
            acc = jnp.where(grp == g, row_max(fold(blk, g)), acc)
        part[pl.ds(NB - 1, 1), :] = to_row(acc)
        ex1.start()
        tail(1).wait()
        m12, m13 = fold(blk, 12), fold(blk, 13)
        tail(2).wait()
        m14 = fold(blk, 14)
        t0, t1 = blk[pl.ds(0, 8), pl.ds(0, 128)], blk[pl.ds(8, 8), pl.ds(0, 128)]
        tail(3).wait()
        m15 = fold(blk, 15)
        c12, c13, c14, c15 = row_max(m12), row_max(m13), row_max(m14), row_max(m15)
        low = negs
        for g, c in ((12, c12), (0, row_max(t0)), (13, c13), (1, row_max(t1))):
            low = jnp.maximum(low, jnp.where(lane == sub + 8 * g, c, NEG))
        for shift in (4, 2, 1) * 3:
            low = jnp.maximum(low, pltpu.roll(low, shift, 0))
        acc = negs
        for g, c in ((14, c14), (15, c15), (12, c12), (13, c13)):
            acc = jnp.where(grp == g, c, acc)
        last_s[...] = to_row(acc)
        ex2.start()

        reread.start()
        reread.wait()
        raw_y.wait_recv()
        acc = negs
        for g in range(RY // 8):
            both = jnp.maximum(fold(xbuf.at[0], g), fold(yraw, g))
            acc = jnp.where(grp == g, row_max(both), acc)
        row0 = to_row(acc)
        for copy in (raw_y, raw_x, fwd_x, back_x):
            copy.wait_send()
        ex0.wait()
        out_ref[pl.ds(0, 8), :] = jnp.maximum(
            jnp.maximum(part[pl.ds(0, 8), :], recv[pl.ds(0, 8), :]), as_row(row0, 0))
        out_ref[pl.ds(8, 7), :] = jnp.maximum(part[pl.ds(8, 7), :], recv[pl.ds(8, 7), :])
        last = jnp.maximum(jnp.maximum(part[pl.ds(NB - 1, 1), :], last_s[...]), low[0:1, :])
        ex1.wait_send()
        ex2.wait_send()
        ex1.wait_recv()
        last = jnp.maximum(last, recv[pl.ds(NB - 1, 1), :])
        ex2.wait_recv()
        lane1 = lax.broadcasted_iota(jnp.int32, (1, 128), 1)
        got = last
        for i in range(128 - K, 128):
            got = jnp.where(lane1 == i, last_r[0, i], got)
        out_ref[pl.ds(NB - 1, 1), :] = jnp.maximum(last, got)

    row = pltpu.VMEM((1, 128), jnp.float32)
    out = pl.pallas_call(
        body,
        out_shape=jax.ShapeDtypeStruct((NB, 128), jnp.float32),
        in_specs=[pl.BlockSpec(memory_space=pl.ANY)],
        out_specs=pl.BlockSpec(memory_space=pltpu.VMEM),
        scratch_shapes=[
            pltpu.VMEM((NB, 128, N), jnp.float32),
            pltpu.VMEM((RY, N), jnp.float32),
            pltpu.VMEM((RX, N), jnp.float32),
            pltpu.SMEM((RF, N), jnp.float32),
            pltpu.VMEM((NB, 128), jnp.float32),
            pltpu.VMEM((NB, 128), jnp.float32),
            row,
            pltpu.SMEM((1, 128), jnp.float32),
            row,
            row,
            pltpu.SemaphoreType.DMA((NG,)),
            pltpu.SemaphoreType.DMA((len(TAIL),)),
            pltpu.SemaphoreType.DMA((2,)),
            pltpu.SemaphoreType.DMA((7,)),
            pltpu.SemaphoreType.DMA((7,)),
            pltpu.SemaphoreType.REGULAR,
        ],
        compiler_params=pltpu.CompilerParams(collective_id=0, disable_semaphore_checks=True),
    )(x.reshape(NB, 128, N))
    return out.reshape(M, 1)
```

```python
import jax
import jax.numpy as jnp
from jax import lax
from jax.experimental import pallas as pl
from jax.experimental.pallas import tpu as pltpu

M, N = 2048, 1024
NB = 16
NEG = float("-inf")
MESH = pl.DeviceIdType.MESH

SW_A = [(8 * b - 1, 8 * b + 7) for b in range(1, 15)] + [(119, 128), (0, 7)]
SW_B = [(16 * b + 7, 16 * b + 23) for b in range(7)] + [(119, 128), (0, 7)]
SW_0 = [(8 * b, 8 * b + 8) for b in range(16)]

def make(SW=SW_B, Y=(7, 119), X=(7, 55), RF=16, EARLY=3, FWD_AFTER=1, X_AFTER=5, T0=0, interpret=False):
    NS = len(SW)
    def inside(r, s): return r[0] <= s[0] and s[1] <= r[1]
    def disjoint(r, s): return s[1] <= r[0] or r[1] <= s[0]
    for s in SW:
        assert inside(Y, s) or disjoint(Y, s); assert inside(X, s) or disjoint(X, s)
        assert not (inside(X, s) and not inside(Y, s))
        assert inside((0, T0), s) or disjoint((0, T0), s)
    first = [int(inside(Y, s)) + int(inside(X, s)) for s in SW]
    lastb = [NB if inside((0, T0), s) else NB - 1 for s in SW]
    TAIL = ((T0, 96), (96, 112), (112, 120), (120, 128))
    K = 32
    NY, NX = Y[1] - Y[0], X[1] - X[0]
    def swept(a):
        return {t for i, s in enumerate(SW) if first[i] <= a < lastb[i] for t in range(*s)}

    def kernel(x):
        def body(x_hbm, out_ref, xbuf, yraw, xraw, stage, part, recv, last_s, last_r, px_s, px_r,
                 sweep_sems, tail_sems, misc_sems, send_sems, recv_sems, ready):
            def rng(r): return pl.ds(r[0], r[1] - r[0])
            def sweep(i):
                idx = (pl.ds(first[i], lastb[i] - first[i]), rng(SW[i]))
                return pltpu.make_async_copy(x_hbm.at[idx], xbuf.at[idx], sweep_sems.at[i])
            def tail(r):
                idx = (NB - 1, rng(TAIL[r]))
                return pltpu.make_async_copy(x_hbm.at[idx], xbuf.at[idx], tail_sems.at[r])
            stage_in = pltpu.make_async_copy(x_hbm.at[1, pl.ds(X[1] - RF, RF)], stage, misc_sems.at[0])
            reread = pltpu.make_async_copy(x_hbm.at[0, rng(Y)], xbuf.at[0, rng(Y)], misc_sems.at[1])

            sweep(0).start()
            stage_in.start()
            for i in range(1, EARLY):
                sweep(i).start()

            mx, my = lax.axis_index("x"), lax.axis_index("y")
            ynbr, xnbr = (mx, 1 - my), (1 - mx, my)
            barrier = pltpu.get_barrier_semaphore()
            pl.semaphore_signal(barrier, inc=1, device_id=ynbr, device_id_type=MESH)

            @pl.when(mx == 0)
            def _():
                pl.semaphore_signal(barrier, inc=1, device_id=xnbr, device_id_type=MESH)
                pl.semaphore_wait(barrier, 1)

            @pl.when(mx == 1)
            def _():
                pl.semaphore_wait(barrier, 2)
                pl.semaphore_signal(ready, inc=1, device_id=xnbr, device_id_type=MESH)

            def remote(i, src, dst, dev):
                return pltpu.make_async_remote_copy(
                    src_ref=src, dst_ref=dst, send_sem=send_sems.at[i], recv_sem=recv_sems.at[i],
                    device_id=dev, device_id_type=MESH)

            raw_y = remote(0, x_hbm.at[0, rng(Y)], yraw, ynbr)
            raw_x = remote(1, x_hbm.at[1, pl.ds(X[0], NX - RF)], xraw.at[pl.ds(0, NX - RF)], xnbr)
            fwd_x = remote(2, stage, xraw.at[pl.ds(NX - RF, RF)], xnbr)
            back_x = remote(3, px_s, px_r, xnbr)
            ex0 = remote(4, part.at[pl.ds(0, NB - 1)], recv.at[pl.ds(0, NB - 1)], ynbr)
            ex1 = remote(5, part.at[pl.ds(NB - 1, 1)], recv.at[pl.ds(NB - 1, 1)], ynbr)
            ex2 = remote(6, last_s, last_r, ynbr)

            raw_y.start()
            for i in range(EARLY, NS):
                sweep(i).start()
            for r in range(len(TAIL)):
                tail(r).start()

            @pl.when(mx == 0)
            def _():
                pl.semaphore_wait(ready, 1)

            raw_x.start()

            lane = lax.broadcasted_iota(jnp.int32, (8, 128), 1)
            sub = lax.broadcasted_iota(jnp.int32, (8, 128), 0)
            grp = lane >> 3
            negs = jnp.full((8, 128), NEG, jnp.float32)

            def fold(v):
                while len(v) > 1:
                    v = [jnp.maximum(v[2 * i], v[2 * i + 1]) for i in range(len(v) // 2)] + v[len(v) // 2 * 2:]
                return v[0]
            def row_max(m):
                return jnp.broadcast_to(jnp.max(m, axis=1, keepdims=True), (8, 128))
            def to_row(acc):
                rs = [acc] + [pltpu.roll(acc, 8 - k, 0) for k in range(1, 8)]
                for bit in (1, 2, 4):
                    odd = (lane & bit) != 0
                    rs = [jnp.where(odd, rs[2 * i + 1], rs[2 * i]) for i in range(len(rs) // 2)]
                return rs[0][0:1, :]
            def to_rows(v):
                for bit in (4, 2, 1):
                    hi = (sub & bit) != 0
                    same = hi == ((lane & bit) != 0)
                    nv = []
                    for a in range(bit):
                        stay = jnp.where(hi, v[a + bit], v[a])
                        move = jnp.where(hi, v[a], v[a + bit])
                        if bit == 4:
                            move = pltpu.roll(move, 4, 0)
                        else:
                            move = jnp.where(hi, pltpu.roll(move, bit, 0), pltpu.roll(move, 8 - bit, 0))
                        nv.append(jnp.where(same, stay, move))
                    v = nv
                return v[0]
            def as_row(row, a):
                return jnp.where(sub == a, jnp.broadcast_to(row, (8, 128)), NEG)

            accs = [negs] * NB
            have = [set() for _ in range(NB)]
            done = [set() for _ in range(NB)]
            for i in range(NS):
                sweep(i).wait()
                if i == NS - 1:
                    back_x.wait_recv()
                for a in range(first[i], lastb[i]):
                    have[a] |= set(range(*SW[i]))
                for g in range(16):
                    for a in range(NB):
                        full = set(range(8 * g, 8 * g + 8))
                        want = (full & swept(a)) if a < NB - 1 else full
                        if want and want <= have[a] and g not in done[a]:
                            done[a].add(g)
                            accs[a] = jnp.where(grp == g, row_max(fold([xbuf[a, t] for t in sorted(want)])), accs[a])
                if i == FWD_AFTER:
                    stage_in.wait()
                    fwd_x.start()
                if i == X_AFTER:
                    raw_x.wait_recv()
                    fwd_x.wait_recv()
                    acc = negs
                    for g in range(16):
                        ts = [t for t in range(8 * g, 8 * g + 8) if X[0] <= t < X[1]]
                        if ts:
                            acc = jnp.where(grp == g, row_max(fold([xraw[t - X[0]] for t in ts])), acc)
                    px_s[...] = to_row(acc)
                    back_x.start()
            part[pl.ds(0, 8), :] = jnp.maximum(to_rows(accs[:8]), as_row(px_r[...], 1))
            part[pl.ds(8, 7), :] = to_rows(accs[8:])[0:7, :]
            ex0.start()

            def grp15(g):
                return fold([xbuf[NB - 1, t] for t in range(8 * g, 8 * g + 8)])
            tail(0).wait()
            acc = accs[NB - 1]
            for g in range(12):
                if g not in done[NB - 1]:
                    acc = jnp.where(grp == g, row_max(grp15(g)), acc)
            part[pl.ds(NB - 1, 1), :] = to_row(acc)
            ex1.start()
            tail(1).wait()
            m12, m13 = grp15(12), grp15(13)
            tail(2).wait()
            m14 = grp15(14)
            t0, t1 = xbuf[NB - 1, 0], xbuf[NB - 1, 8]
            tail(3).wait()
            m15 = grp15(15)
            c12, c13, c14, c15 = row_max(m12), row_max(m13), row_max(m14), row_max(m15)
            low = negs
            for g, c in ((12, c12), (0, row_max(t0)), (13, c13), (1, row_max(t1))):
                low = jnp.maximum(low, jnp.where(lane == sub + 8 * g, c, NEG))
            for shift in (4, 2, 1) * 3:
                low = jnp.maximum(low, pltpu.roll(low, shift, 0))
            acc = negs
            for g, c in ((14, c14), (15, c15), (12, c12), (13, c13)):
                acc = jnp.where(grp == g, c, acc)
            last_s[...] = to_row(acc)
            ex2.start()

            reread.start()
            reread.wait()
            raw_y.wait_recv()
            acc = negs
            for g in range(16):
                ts = [t for t in range(8 * g, 8 * g + 8) if Y[0] <= t < Y[1]]
                if ts:
                    acc = jnp.where(grp == g, row_max(fold([xbuf[0, t] for t in ts] + [yraw[t - Y[0]] for t in ts])), acc)
            row0 = to_row(acc)
            for copy in (raw_y, raw_x, fwd_x, back_x):
                copy.wait_send()
            ex0.wait()
            out_ref[pl.ds(0, 8), :] = jnp.maximum(
                jnp.maximum(part[pl.ds(0, 8), :], recv[pl.ds(0, 8), :]), as_row(row0, 0))
            out_ref[pl.ds(8, 7), :] = jnp.maximum(part[pl.ds(8, 7), :], recv[pl.ds(8, 7), :])
            last = jnp.maximum(jnp.maximum(part[pl.ds(NB - 1, 1), :], last_s[...]), low[0:1, :])
            ex1.wait_send()
            ex2.wait_send()
            ex1.wait_recv()
            last = jnp.maximum(last, recv[pl.ds(NB - 1, 1), :])
            ex2.wait_recv()
            lane1 = lax.broadcasted_iota(jnp.int32, (1, 128), 1)
            got = last
            for i in range(128 - K, 128):
                got = jnp.where(lane1 == i, last_r[0, i], got)
            out_ref[pl.ds(NB - 1, 1), :] = jnp.maximum(last, got)

        row = pltpu.VMEM((1, 128), jnp.float32)
        xt = x.reshape(256, 8, 8, 128).transpose(0, 2, 1, 3).reshape(NB, 128, 8, 128)
        out = pl.pallas_call(
            body,
            out_shape=jax.ShapeDtypeStruct((NB, 128), jnp.float32),
            in_specs=[pl.BlockSpec(memory_space=pl.ANY)],
            out_specs=pl.BlockSpec(memory_space=pltpu.VMEM),
            scratch_shapes=[
                pltpu.VMEM((NB, 128, 8, 128), jnp.float32),
                pltpu.VMEM((NY, 8, 128), jnp.float32),
                pltpu.VMEM((NX, 8, 128), jnp.float32),
                pltpu.SMEM((RF, 8, 128), jnp.float32),
                pltpu.VMEM((NB, 128), jnp.float32),
                pltpu.VMEM((NB, 128), jnp.float32),
                row,
                pltpu.SMEM((1, 128), jnp.float32),
                row, row,
                pltpu.SemaphoreType.DMA((NS,)),
                pltpu.SemaphoreType.DMA((len(TAIL),)),
                pltpu.SemaphoreType.DMA((2,)),
                pltpu.SemaphoreType.DMA((7,)),
                pltpu.SemaphoreType.DMA((7,)),
                pltpu.SemaphoreType.REGULAR,
            ],
            compiler_params=pltpu.CompilerParams(collective_id=0, disable_semaphore_checks=True),
            interpret=interpret,
        )(xt)
        return out.reshape(M, 1)
    return kernel

pallas_dist_max_ax1_xy_m2048_n1024_kernel = make(SW=SW_B[:3]+SW_B[7:]+SW_B[3:7],X_AFTER=6)
```

```python
import jax
import jax.numpy as jnp
from jax import lax
from jax.experimental import pallas as pl
from jax.experimental.pallas import tpu as pltpu

M, N = 2048, 1024
NB = 16
NEG = float("-inf")
MESH = pl.DeviceIdType.MESH

Y = (15, 7, 112)
X = (14, 7, 32)
NF = 16

STAGES = [
    [(0, 14, 7, 16)],
    [(0, 14, 23, 16)],
    [(0, 15, 39, 16)],
    [(0, 16, 119, 9), (0, 16, 0, 7)],
    [(0, 15, 55, 16)],
    [(0, 15, 71, 16)],
    [(0, 15, 87, 16), (13, 2, 103, 1)],
]
PARTS = [(0, 8, 103, 16), (8, 3, 103, 16), (11, 2, 103, 16)]
TAIL = [(13, 1, 104, 15), (14, 1, 104, 8), (14, 1, 112, 7)]
LOADS = [d for stage in STAGES for d in stage] + PARTS + TAIL
MSGS = [(13, 3)] + [d[:2] for d in PARTS]
EARLY = 2
FWD_AFTER = 1
X_AFTER = 4


def _tiles(d):
    return {(a, t) for a in range(d[0], d[0] + d[1]) for t in range(d[2], d[2] + d[3])}


MAIN = set().union(*map(_tiles, LOADS))
assert len(MAIN) == sum(d[1] * d[3] for d in LOADS)
assert MAIN | _tiles((Y[0], 1) + Y[1:]) | _tiles((X[0], 1) + X[1:]) == _tiles((0, NB, 0, 128))


def pallas_dist_max_ax1_xy_m2048_n1024_kernel(x: jax.Array):
    def body(x_hbm, out_ref, xbuf, yraw, xraw, stage, part, recv, last_s, last_r, px_s, px_r,
             load_sems, misc_sems, send_sems, recv_sems, ready):
        def load(d):
            idx = (pl.ds(d[0], d[1]), pl.ds(d[2], d[3]))
            return pltpu.make_async_copy(x_hbm.at[idx], xbuf.at[idx], load_sems.at[LOADS.index(d)])

        y_idx = (Y[0], pl.ds(Y[1], Y[2]))
        nd = X[2] - NF
        stage_in = pltpu.make_async_copy(x_hbm.at[X[0], pl.ds(X[1] + nd, NF)], stage, misc_sems.at[0])
        reread = pltpu.make_async_copy(x_hbm.at[y_idx], xbuf.at[y_idx], misc_sems.at[1])

        load(LOADS[0]).start()
        stage_in.start()
        for d in LOADS[1:EARLY]:
            load(d).start()

        mx, my = lax.axis_index("x"), lax.axis_index("y")
        ynbr, xnbr = (mx, 1 - my), (1 - mx, my)
        barrier = pltpu.get_barrier_semaphore()
        pl.semaphore_signal(barrier, inc=1, device_id=ynbr, device_id_type=MESH)

        @pl.when(mx == 0)
        def _():
            pl.semaphore_signal(barrier, inc=1, device_id=xnbr, device_id_type=MESH)
            pl.semaphore_wait(barrier, 1)

        @pl.when(mx == 1)
        def _():
            pl.semaphore_wait(barrier, 2)
            pl.semaphore_signal(ready, inc=1, device_id=xnbr, device_id_type=MESH)

        def remote(i, src, dst, dev):
            return pltpu.make_async_remote_copy(
                src_ref=src, dst_ref=dst, send_sem=send_sems.at[i], recv_sem=recv_sems.at[i],
                device_id=dev, device_id_type=MESH)

        raw_y = remote(0, x_hbm.at[y_idx], yraw, ynbr)
        raw_x = remote(1, x_hbm.at[X[0], pl.ds(X[1], nd)], xraw.at[pl.ds(0, nd)], xnbr)
        fwd_x = remote(2, stage, xraw.at[pl.ds(nd, NF)], xnbr)
        back_x = remote(3, px_s, px_r, xnbr)
        final = remote(4, last_s, last_r, ynbr)
        msgs = [remote(5 + i, part.at[pl.ds(*m)], recv.at[pl.ds(*m)], ynbr) for i, m in enumerate(MSGS)]

        raw_y.start()
        for d in LOADS[EARLY:]:
            load(d).start()

        @pl.when(mx == 0)
        def _():
            pl.semaphore_wait(ready, 1)

        raw_x.start()

        lane = lax.broadcasted_iota(jnp.int32, (8, 128), 1)
        sub = lax.broadcasted_iota(jnp.int32, (8, 128), 0)
        grp = lane >> 3
        negs = jnp.full((8, 128), NEG, jnp.float32)

        def fold(v):
            while len(v) > 1:
                half = len(v) // 2
                v = [jnp.maximum(v[2 * i], v[2 * i + 1]) for i in range(half)] + v[2 * half:]
            return v[0]

        def row_max(m):
            return jnp.broadcast_to(jnp.max(m, axis=1, keepdims=True), (8, 128))

        def to_row(acc):
            rs = [acc] + [pltpu.roll(acc, 8 - k, 0) for k in range(1, 8)]
            for bit in (1, 2, 4):
                odd = (lane & bit) != 0
                rs = [jnp.where(odd, rs[2 * i + 1], rs[2 * i]) for i in range(len(rs) // 2)]
            return rs[0][0:1, :]

        def to_rows(v):
            for bit in (4, 2, 1):
                hi = (sub & bit) != 0
                same = hi == ((lane & bit) != 0)
                nv = []
                for a in range(bit):
                    stay = jnp.where(hi, v[a + bit], v[a])
                    move = jnp.where(hi, v[a], v[a + bit])
                    if bit == 4:
                        move = pltpu.roll(move, 4, 0)
                    else:
                        move = jnp.where(hi, pltpu.roll(move, bit, 0), pltpu.roll(move, 8 - bit, 0))
                    nv.append(jnp.where(same, stay, move))
                v = nv
            return v[0]

        def as_row(row, a):
            return jnp.where(sub == a % 8, jnp.broadcast_to(row, (8, 128)), NEG)

        def raw_row(first, count, get):
            acc = negs
            for g in range(16):
                ts = [t for t in range(8 * g, 8 * g + 8) if first <= t < first + count]
                if ts:
                    acc = jnp.where(grp == g, row_max(fold(get(ts))), acc)
            return to_row(acc)

        accs = [negs] * NB
        have, done = set(), set()

        def wait(loads):
            for d in loads:
                load(d).wait()
                have.update(_tiles(d))

        def reduce_complete_groups():
            for g in range(16):
                for a in range(NB):
                    want = _tiles((a, 1, 8 * g, 8)) & MAIN
                    if want and want <= have and (a, g) not in done:
                        done.add((a, g))
                        m = fold([xbuf[t] for t in sorted(want)])
                        accs[a] = jnp.where(grp == g, row_max(m), accs[a])

        def send_rows(i):
            first, count = MSGS[i]
            if count == 8:
                part[pl.ds(first, 8), :] = to_rows(accs[first:first + 8])
            else:
                for a in range(first, first + count):
                    row = to_row(accs[a])
                    part[pl.ds(a, 1), :] = jnp.maximum(row, px_r[...]) if a == X[0] else row
            msgs[i].start()

        for i, loads in enumerate(STAGES):
            wait(loads)
            if i == len(STAGES) - 1:
                back_x.wait_recv()
            reduce_complete_groups()
            if i == FWD_AFTER:
                stage_in.wait()
                fwd_x.start()
            if i == X_AFTER:
                raw_x.wait_recv()
                fwd_x.wait_recv()
                px_s[...] = raw_row(X[1], X[2], lambda ts: [xraw[t - X[1]] for t in ts])
                back_x.start()
        send_rows(0)
        for i, d in enumerate(PARTS):
            wait([d])
            reduce_complete_groups()
            send_rows(i + 1)

        def group(a, g):
            return fold([xbuf[a, t] for t in range(8 * g, 8 * g + 8)])

        load(TAIL[0]).wait()
        ma, mb = group(13, 13), group(13, 14)
        load(TAIL[1]).wait()
        mc = group(14, 13)
        t0, t1 = xbuf[13, 0], xbuf[13, 8]
        load(TAIL[2]).wait()
        md = group(14, 14)
        ca, cb, cc, cd = row_max(ma), row_max(mb), row_max(mc), row_max(md)
        row13 = negs
        for g, c in ((13, ca), (0, row_max(t0)), (14, cb), (1, row_max(t1))):
            row13 = jnp.maximum(row13, jnp.where(lane == sub + 8 * g, c, NEG))
        for shift in (4, 2, 1) * 3:
            row13 = jnp.maximum(row13, pltpu.roll(row13, shift, 0))
        acc = negs
        for g, c in ((2, cc), (3, cd), (0, ca), (1, cb)):
            acc = jnp.where(grp == g, c, acc)
        last_s[...] = to_row(acc)
        final.start()

        reread.start()
        row14 = to_row(jnp.where(grp == 13, cc, jnp.where(grp == 14, cd, NEG)))
        hi = jnp.maximum(jnp.where(sub == 13 % 8, row13, NEG), as_row(row14, 14))
        reread.wait()
        raw_y.wait_recv()
        row15 = raw_row(
            Y[1], Y[2], lambda ts: [xbuf[Y[0], t] for t in ts] + [yraw[t - Y[1]] for t in ts])
        hi = jnp.maximum(hi, as_row(row15, Y[0]))
        for copy in (raw_y, raw_x, fwd_x, back_x):
            copy.wait_send()
        for msg in msgs[:-1]:
            msg.wait()
        out_ref[pl.ds(0, 8), :] = jnp.maximum(part[pl.ds(0, 8), :], recv[pl.ds(0, 8), :])
        hi = jnp.maximum(hi, part[pl.ds(8, 8), :])
        msgs[-1].wait_send()
        final.wait_send()
        msgs[-1].wait_recv()
        hi = jnp.maximum(hi, recv[pl.ds(8, 8), :])
        final.wait_recv()
        pos = sub * 128 + lane
        got = hi
        for i in range(32):
            got = jnp.where(pos == (13 + i // 16) % 8 * 128 + 104 + i % 16, last_r[0, i], got)
        out_ref[pl.ds(8, 8), :] = jnp.maximum(hi, got)

    row = pltpu.VMEM((1, 128), jnp.float32)
    tiled = x.reshape(M // 8, 8, N // 128, 128).transpose(0, 2, 1, 3).reshape(NB, 128, 8, 128)
    out = pl.pallas_call(
        body,
        out_shape=jax.ShapeDtypeStruct((NB, 128), jnp.float32),
        in_specs=[pl.BlockSpec(memory_space=pl.ANY)],
        out_specs=pl.BlockSpec(memory_space=pltpu.VMEM),
        scratch_shapes=[
            pltpu.VMEM((NB, 128, 8, 128), jnp.float32),
            pltpu.VMEM((Y[2], 8, 128), jnp.float32),
            pltpu.VMEM((X[2], 8, 128), jnp.float32),
            pltpu.SMEM((NF, 8, 128), jnp.float32),
            pltpu.VMEM((NB, 128), jnp.float32),
            pltpu.VMEM((NB, 128), jnp.float32),
            row,
            pltpu.SMEM((1, 128), jnp.float32),
            row,
            row,
            pltpu.SemaphoreType.DMA((len(LOADS),)),
            pltpu.SemaphoreType.DMA((2,)),
            pltpu.SemaphoreType.DMA((5 + len(MSGS),)),
            pltpu.SemaphoreType.DMA((5 + len(MSGS),)),
            pltpu.SemaphoreType.REGULAR,
        ],
        compiler_params=pltpu.CompilerParams(collective_id=0, disable_semaphore_checks=True),
    )(tiled)
    return out.reshape(M, 1)
```

```python
import jax
import jax.numpy as jnp
from jax import lax
from jax.experimental import pallas as pl
from jax.experimental.pallas import tpu as pltpu

M, N = 2048, 1024
NB = 16
NEG = float("-inf")
MESH = pl.DeviceIdType.MESH

Y = (15, 7, 112)
X = (14, 7, 32)
NF = 16

STAGES = [
    [(0, 14, 7, 16)],
    [(0, 14, 23, 16)],
    [(0, 15, 39, 16)],
    [(0, 16, 119, 9), (0, 16, 0, 7)],
    [(0, 15, 55, 16)],
    [(0, 15, 71, 16)],
    [(0, 15, 87, 16), (13, 2, 103, 1)],
]
PARTS = [(0, 8, 103, 16), (8, 3, 103, 16), (11, 2, 103, 16)]
TAIL = [(13, 1, 104, 15), (14, 1, 104, 8), (14, 1, 112, 7)]
LOADS = [d for stage in STAGES for d in stage] + PARTS + TAIL
MSGS = [(13, 3)] + [d[:2] for d in PARTS]
EARLY = 2
FWD_AFTER = 1
Y_AFTER = 3
X_AFTER = 4


def _tiles(d):
    return {(a, t) for a in range(d[0], d[0] + d[1]) for t in range(d[2], d[2] + d[3])}


MAIN = set().union(*map(_tiles, LOADS))
assert len(MAIN) == sum(d[1] * d[3] for d in LOADS)
assert MAIN | _tiles((Y[0], 1) + Y[1:]) | _tiles((X[0], 1) + X[1:]) == _tiles((0, NB, 0, 128))


def pallas_dist_max_ax1_xy_m2048_n1024_kernel(x: jax.Array):
    def body(x_hbm, out_ref, xbuf, yraw, xraw, stage, part, recv, last_s, last_r, px_s, px_r, py,
             load_sems, misc_sems, send_sems, recv_sems, ready):
        def load(d):
            idx = (pl.ds(d[0], d[1]), pl.ds(d[2], d[3]))
            return pltpu.make_async_copy(x_hbm.at[idx], xbuf.at[idx], load_sems.at[LOADS.index(d)])

        y_idx = (Y[0], pl.ds(Y[1], Y[2]))
        nd = X[2] - NF
        stage_in = pltpu.make_async_copy(x_hbm.at[X[0], pl.ds(X[1] + nd, NF)], stage, misc_sems.at[0])
        early_y = pltpu.make_async_copy(x_hbm.at[y_idx], xbuf.at[y_idx], misc_sems.at[1])
        late_y = pltpu.make_async_copy(x_hbm.at[y_idx], yraw, misc_sems.at[2])

        load(LOADS[0]).start()
        stage_in.start()
        for d in LOADS[1:EARLY]:
            load(d).start()

        mx, my = lax.axis_index("x"), lax.axis_index("y")
        ynbr, xnbr = (mx, 1 - my), (1 - mx, my)
        barrier = pltpu.get_barrier_semaphore()
        pl.semaphore_signal(barrier, inc=1, device_id=ynbr, device_id_type=MESH)

        @pl.when(mx == 0)
        def _():
            pl.semaphore_signal(barrier, inc=1, device_id=xnbr, device_id_type=MESH)
            pl.semaphore_wait(barrier, 1)

        @pl.when(mx == 1)
        def _():
            pl.semaphore_wait(barrier, 2)
            pl.semaphore_signal(ready, inc=1, device_id=xnbr, device_id_type=MESH)

        def remote(i, src, dst, dev):
            return pltpu.make_async_remote_copy(
                src_ref=src, dst_ref=dst, send_sem=send_sems.at[i], recv_sem=recv_sems.at[i],
                device_id=dev, device_id_type=MESH)

        raw_y = remote(0, x_hbm.at[y_idx], yraw, ynbr)
        raw_x = remote(1, x_hbm.at[X[0], pl.ds(X[1], nd)], xraw.at[pl.ds(0, nd)], xnbr)
        fwd_x = remote(2, stage, xraw.at[pl.ds(nd, NF)], xnbr)
        back_x = remote(3, px_s, px_r, xnbr)
        final = remote(4, last_s, last_r, ynbr)
        msgs = [remote(5 + i, part.at[pl.ds(*m)], recv.at[pl.ds(*m)], ynbr) for i, m in enumerate(MSGS)]

        pl.when(my == 1)(raw_y.start)
        pl.when(my == 0)(early_y.start)
        for d in LOADS[EARLY:]:
            load(d).start()

        @pl.when(mx == 0)
        def _():
            pl.semaphore_wait(ready, 1)

        raw_x.start()

        lane = lax.broadcasted_iota(jnp.int32, (8, 128), 1)
        sub = lax.broadcasted_iota(jnp.int32, (8, 128), 0)
        grp = lane >> 3
        negs = jnp.full((8, 128), NEG, jnp.float32)

        def fold(v):
            while len(v) > 1:
                half = len(v) // 2
                v = [jnp.maximum(v[2 * i], v[2 * i + 1]) for i in range(half)] + v[2 * half:]
            return v[0]

        def row_max(m):
            return jnp.broadcast_to(jnp.max(m, axis=1, keepdims=True), (8, 128))

        def to_row(acc):
            rs = [acc] + [pltpu.roll(acc, 8 - k, 0) for k in range(1, 8)]
            for bit in (1, 2, 4):
                odd = (lane & bit) != 0
                rs = [jnp.where(odd, rs[2 * i + 1], rs[2 * i]) for i in range(len(rs) // 2)]
            return rs[0][0:1, :]

        def to_rows(v):
            for bit in (4, 2, 1):
                hi = (sub & bit) != 0
                same = hi == ((lane & bit) != 0)
                nv = []
                for a in range(bit):
                    stay = jnp.where(hi, v[a + bit], v[a])
                    move = jnp.where(hi, v[a], v[a + bit])
                    if bit == 4:
                        move = pltpu.roll(move, 4, 0)
                    else:
                        move = jnp.where(hi, pltpu.roll(move, bit, 0), pltpu.roll(move, 8 - bit, 0))
                    nv.append(jnp.where(same, stay, move))
                v = nv
            return v[0]

        def as_row(row, a):
            return jnp.where(sub == a % 8, jnp.broadcast_to(row, (8, 128)), NEG)

        def raw_row(first, count, get):
            acc = negs
            for g in range(16):
                ts = [t for t in range(8 * g, 8 * g + 8) if first <= t < first + count]
                if ts:
                    acc = jnp.where(grp == g, row_max(fold(get(ts))), acc)
            return to_row(acc)

        accs = [negs] * NB
        have, done = set(), set()

        def wait(loads):
            for d in loads:
                load(d).wait()
                have.update(_tiles(d))

        def reduce_complete_groups():
            for g in range(16):
                for a in range(NB):
                    want = _tiles((a, 1, 8 * g, 8)) & MAIN
                    if want and want <= have and (a, g) not in done:
                        done.add((a, g))
                        m = fold([xbuf[t] for t in sorted(want)])
                        accs[a] = jnp.where(grp == g, row_max(m), accs[a])

        def send_rows(i):
            first, count = MSGS[i]
            if count == 8:
                part[pl.ds(first, 8), :] = to_rows(accs[first:first + 8])
            else:
                for a in range(first, first + count):
                    row = to_row(accs[a])
                    if a in (X[0], Y[0]):
                        row = jnp.maximum(row, (px_r if a == X[0] else py)[...])
                    part[pl.ds(a, 1), :] = row
            msgs[i].start()

        for i, loads in enumerate(STAGES):
            wait(loads)
            if i == len(STAGES) - 1:
                back_x.wait_recv()
            reduce_complete_groups()
            if i == FWD_AFTER:
                stage_in.wait()
                fwd_x.start()
            if i == Y_AFTER:
                py[...] = negs[0:1, :]

                @pl.when(my == 0)
                def _():
                    early_y.wait()
                    py[...] = raw_row(Y[1], Y[2], lambda ts: [xbuf[Y[0], t] for t in ts])
            if i == X_AFTER:
                raw_x.wait_recv()
                fwd_x.wait_recv()
                px_s[...] = raw_row(X[1], X[2], lambda ts: [xraw[t - X[1]] for t in ts])
                back_x.start()
        send_rows(0)
        for i, d in enumerate(PARTS):
            wait([d])
            reduce_complete_groups()
            send_rows(i + 1)

        def group(a, g):
            return fold([xbuf[a, t] for t in range(8 * g, 8 * g + 8)])

        load(TAIL[0]).wait()
        ma, mb = group(13, 13), group(13, 14)
        load(TAIL[1]).wait()
        mc = group(14, 13)
        t0, t1 = xbuf[13, 0], xbuf[13, 8]
        for t in range(1, 8):
            t0 = jnp.maximum(t0, xbuf[13, t])
        load(TAIL[2]).wait()
        md = group(14, 14)
        ca, cb, cc, cd = row_max(ma), row_max(mb), row_max(mc), row_max(md)
        row13 = negs
        for g, c in ((13, ca), (0, row_max(t0)), (14, cb), (1, row_max(t1))):
            row13 = jnp.maximum(row13, jnp.where(lane == sub + 8 * g, c, NEG))
        for shift in (4, 2, 1) * 3:
            row13 = jnp.maximum(row13, pltpu.roll(row13, shift, 0))
        acc = negs
        for g, c in ((2, cc), (0, ca), (1, cb), (3, cd)):
            acc = jnp.where(grp == g, c, acc)
        last_s[...] = to_row(acc)
        final.start()

        pl.when(my == 1)(late_y.start)
        row14 = to_row(jnp.where(grp == 13, cc, jnp.where(grp == 14, cd, NEG)))
        hi = jnp.maximum(jnp.where(sub == 13 % 8, row13, NEG), as_row(row14, 14))

        @pl.when(my == 1)
        def _():
            late_y.wait()
            raw_y.wait_send()

        pl.when(my == 0)(raw_y.wait_recv)
        row15 = raw_row(Y[1], Y[2], lambda ts: [yraw[t - Y[1]] for t in ts])
        hi = jnp.maximum(hi, as_row(row15, Y[0]))
        for copy in (raw_x, fwd_x, back_x):
            copy.wait_send()
        for msg in msgs[:-1]:
            msg.wait()
        out_ref[pl.ds(0, 8), :] = jnp.maximum(part[pl.ds(0, 8), :], recv[pl.ds(0, 8), :])
        hi = jnp.maximum(hi, part[pl.ds(8, 8), :])
        msgs[-1].wait_send()
        final.wait_send()
        msgs[-1].wait_recv()
        hi = jnp.maximum(hi, recv[pl.ds(8, 8), :])
        final.wait_recv()
        pos = sub * 128 + lane
        got = hi
        for i in range(32):
            got = jnp.where(pos == (13 + i // 16) % 8 * 128 + 104 + i % 16, last_r[0, i], got)
        out_ref[pl.ds(8, 8), :] = jnp.maximum(hi, got)

    row = pltpu.VMEM((1, 128), jnp.float32)
    tiled = x.reshape(M // 8, 8, N // 128, 128).transpose(0, 2, 1, 3).reshape(NB, 128, 8, 128)
    out = pl.pallas_call(
        body,
        out_shape=jax.ShapeDtypeStruct((NB, 128), jnp.float32),
        in_specs=[pl.BlockSpec(memory_space=pl.ANY)],
        out_specs=pl.BlockSpec(memory_space=pltpu.VMEM),
        scratch_shapes=[
            pltpu.VMEM((NB, 128, 8, 128), jnp.float32),
            pltpu.VMEM((Y[2], 8, 128), jnp.float32),
            pltpu.VMEM((X[2], 8, 128), jnp.float32),
            pltpu.SMEM((NF, 8, 128), jnp.float32),
            pltpu.VMEM((NB, 128), jnp.float32),
            pltpu.VMEM((NB, 128), jnp.float32),
            row,
            pltpu.SMEM((1, 128), jnp.float32),
            row,
            row,
            row,
            pltpu.SemaphoreType.DMA((len(LOADS),)),
            pltpu.SemaphoreType.DMA((3,)),
            pltpu.SemaphoreType.DMA((5 + len(MSGS),)),
            pltpu.SemaphoreType.DMA((5 + len(MSGS),)),
            pltpu.SemaphoreType.REGULAR,
        ],
        compiler_params=pltpu.CompilerParams(collective_id=0, disable_semaphore_checks=True),
    )(tiled)
    return out.reshape(M, 1)
```
